```python
import numpy as np

kernel_name = "dist_sum_ax0_xy_m2048_n1024"

def setup_inputs():
    return {"x": np.random.randn(4096, 2048).astype(np.float32)}

def reference(x: np.ndarray) -> np.ndarray:
    return np.sum(x, axis=0, keepdims=True)
```

```python
import jax
import jax.numpy as jnp
from jax import lax
from jax.experimental import pallas as pl
from jax.experimental.pallas import tpu as pltpu

_NS = 8
_RP = 8
_NW = 128
_DEPTH = 16
_PRIO = (1, 1, 1, 0, 1, 1, 1, 0)


def _tree_sum(parts):
    parts = list(parts)
    while len(parts) > 1:
        nxt = [parts[i] + parts[i + 1] for i in range(0, len(parts) - 1, 2)]
        if len(parts) % 2:
            nxt.append(parts[-1])
        parts = nxt
    return parts[0]


def pallas_dist_sum_ax0_xy_m2048_n1024_kernel(x: jax.Array):
    m, n = x.shape
    srows = m // _NS
    ng = srows // _RP
    grows = _NS * _RP
    frows = grows - _RP
    wide = n - _NW
    depth = min(_DEPTH, ng)

    def body(x_hbm, out_ref, buf, nbuf, send_buf, recv_buf,
             sems, nsem, send_sems, recv_sems):
        my_x = lax.axis_index("x")
        my_y = lax.axis_index("y")
        peer = (1 - my_x, my_y)

        def issue(g):
            for s in range(_NS):
                w = wide if s == _NS - 1 else n
                src = pl.multiple_of(s * srows + g * _RP, _RP)
                dst = pl.multiple_of(g * grows + s * _RP, _RP)
                pltpu.make_async_copy(
                    x_hbm.at[pl.ds(src, _RP), pl.ds(0, w)],
                    buf.at[pl.ds(dst, _RP), pl.ds(0, w)],
                    sems.at[g],
                ).start(priority=_PRIO[s])

        def consume(g, carry):
            acc_w, acc_n = carry
            r0 = pl.multiple_of(g * grows, grows)
            full = buf.at[pl.ds(r0, frows), :]
            pltpu.make_async_copy(full, full, sems.at[g]).wait()
            rest = buf.at[pl.ds(r0 + frows, _RP), pl.ds(0, wide)]
            pltpu.make_async_copy(rest, rest, sems.at[g]).wait()
            blk_w = buf[pl.ds(r0, grows), pl.ds(0, wide)]
            blk_n = buf[pl.ds(r0, frows), pl.ds(wide, _NW)]
            acc_w = acc_w + blk_w.reshape(_NS, _RP, wide).sum(axis=0)
            acc_n = acc_n + blk_n.reshape(_NS - 1, _RP, _NW).sum(axis=0)
            return acc_w, acc_n

        def exchange(k, c0, w):
            return pltpu.make_async_remote_copy(
                src_ref=send_buf.at[:, pl.ds(c0, w)],
                dst_ref=recv_buf.at[:, pl.ds(c0, w)],
                send_sem=send_sems.at[k],
                recv_sem=recv_sems.at[k],
                device_id=peer,
                device_id_type=pl.DeviceIdType.MESH,
            )

        issue(0)
        bar = pltpu.get_barrier_semaphore()
        pl.semaphore_signal(bar, inc=1, device_id=peer,
                            device_id_type=pl.DeviceIdType.MESH)

        def prologue(g, c):
            issue(g)
            return c

        lax.fori_loop(1, depth, prologue, 0)

        def steady(g, carry):
            issue(g + depth)
            return consume(g, carry)

        carry = (jnp.zeros((_RP, wide), jnp.float32),
                 jnp.zeros((_RP, _NW), jnp.float32))
        carry = lax.fori_loop(0, ng - depth, steady, carry)

        strip = pltpu.make_async_copy(
            x_hbm.at[pl.ds(m - srows, srows), pl.ds(wide, _NW)], nbuf, nsem)
        strip.start(priority=1)

        pl.semaphore_wait(bar, 1)

        acc_w, acc_n = lax.fori_loop(ng - depth, ng, consume, carry)
        send_buf[:, pl.ds(0, wide)] = jnp.sum(acc_w, axis=0, keepdims=True)
        rd_w = exchange(0, 0, wide)
        rd_w.start()

        strip.wait()
        acc_n = _tree_sum(
            [acc_n] + [nbuf[pl.ds(j * _RP, _RP), :] for j in range(ng)])
        part_n = jnp.sum(acc_n, axis=0, keepdims=True)
        send_buf[:, pl.ds(wide, _NW)] = part_n
        rd_n = exchange(1, wide, _NW)
        rd_n.start()

        rd_w.wait_send()
        rd_n.wait_send()
        rd_w.wait_recv()
        out_ref[:, pl.ds(0, wide)] = (
            send_buf[:, pl.ds(0, wide)] + recv_buf[:, pl.ds(0, wide)])
        rd_n.wait_recv()
        out_ref[:, pl.ds(wide, _NW)] = part_n + recv_buf[:, pl.ds(wide, _NW)]

    return pl.pallas_call(
        body,
        out_shape=jax.ShapeDtypeStruct((1, n), jnp.float32),
        in_specs=[pl.BlockSpec(memory_space=pl.ANY)],
        out_specs=pl.BlockSpec(memory_space=pltpu.VMEM),
        scratch_shapes=[
            pltpu.VMEM((m, n), jnp.float32),
            pltpu.VMEM((srows, _NW), jnp.float32),
            pltpu.VMEM((1, n), jnp.float32),
            pltpu.VMEM((1, n), jnp.float32),
            pltpu.SemaphoreType.DMA((ng,)),
            pltpu.SemaphoreType.DMA,
            pltpu.SemaphoreType.DMA((2,)),
            pltpu.SemaphoreType.DMA((2,)),
        ],
        compiler_params=pltpu.CompilerParams(
            collective_id=0,
            disable_semaphore_checks=True,
            disable_bounds_checks=True,
        ),
    )(x)
```

```python
import jax
import jax.numpy as jnp
from jax import lax
from jax.experimental import pallas as pl
from jax.experimental.pallas import tpu as pltpu

_NS = 8
_RP = 8
_NW = 128
_DEPTH = 16
_CHAINS = 6


def _chain_sum(parts):
    accs = list(parts[:_CHAINS])
    for i, p in enumerate(parts[_CHAINS:]):
        accs[i % _CHAINS] = accs[i % _CHAINS] + p
    while len(accs) > 1:
        nxt = [accs[i] + accs[i + 1] for i in range(0, len(accs) - 1, 2)]
        if len(accs) % 2:
            nxt.append(accs[-1])
        accs = nxt
    return accs[0]


def pallas_dist_sum_ax0_xy_m2048_n1024_kernel(x: jax.Array):
    m, n = x.shape
    srows = m // _NS
    ng = srows // _RP
    grows = _NS * _RP
    frows = grows - _RP
    wide = n - _NW
    assert m % (_NS * _RP) == 0 and wide == (_NS - 1) * _NW
    depth = min(_DEPTH, ng)

    def body(x_hbm, out_ref, buf, nbuf, send_w, recv_w, send_n, recv_n,
             sems_p, sems_t, strip_sem, send_sems, recv_sems):

        def issue(g, c):
            r = pl.multiple_of(g * _RP, _RP)
            d = pl.multiple_of(g * grows, grows)
            for s in range(_NS - 1):
                pltpu.make_async_copy(
                    x_hbm.at[pl.ds(m - srows + r, _RP), pl.ds(s * _NW, _NW)],
                    buf.at[pl.ds(d + frows, _RP), pl.ds(s * _NW, _NW)],
                    sems_t.at[g],
                ).start(priority=0)
                pltpu.make_async_copy(
                    x_hbm.at[pl.ds(s * srows + r, _RP), :],
                    buf.at[pl.ds(d + s * _RP, _RP), :],
                    sems_p.at[g],
                ).start(priority=1)
            return c

        def consume(g, carry):
            acc_w, acc_n = carry
            d = pl.multiple_of(g * grows, grows)
            tiles = buf.at[pl.ds(d + frows, _RP), pl.ds(0, wide)]
            pltpu.make_async_copy(tiles, tiles, sems_t.at[g]).wait()
            pieces = buf.at[pl.ds(d, frows), :]
            pltpu.make_async_copy(pieces, pieces, sems_p.at[g]).wait()
            blk_w = buf[pl.ds(d, grows), pl.ds(0, wide)]
            blk_n = buf[pl.ds(d, frows), pl.ds(wide, _NW)]
            acc_w = acc_w + blk_w.reshape(_NS, _RP, wide).sum(axis=0)
            acc_n = acc_n + blk_n.reshape(_NS - 1, _RP, _NW).sum(axis=0)
            return acc_w, acc_n

        lax.fori_loop(0, 2, issue, 0)

        peer = (1 - lax.axis_index("x"), lax.axis_index("y"))
        bar = pltpu.get_barrier_semaphore()
        pl.semaphore_signal(bar, inc=1, device_id=peer,
                            device_id_type=pl.DeviceIdType.MESH)

        lax.fori_loop(2, depth, issue, 0)

        def steady(g, carry):
            issue(g + depth, 0)
            return consume(g, carry)

        carry = (jnp.zeros((_RP, wide), jnp.float32),
                 jnp.zeros((_RP, _NW), jnp.float32))
        carry = lax.fori_loop(0, ng - depth, steady, carry)

        strip = pltpu.make_async_copy(
            x_hbm.at[pl.ds(m - srows, srows), pl.ds(wide, _NW)],
            nbuf, strip_sem)
        strip.start(priority=1)

        pl.semaphore_wait(bar, 1)

        def exchange(k, src, dst):
            return pltpu.make_async_remote_copy(
                src_ref=src, dst_ref=dst,
                send_sem=send_sems.at[k], recv_sem=recv_sems.at[k],
                device_id=peer, device_id_type=pl.DeviceIdType.MESH,
            )

        acc_w, acc_n = lax.fori_loop(ng - depth, ng, consume, carry)
        send_w[...] = jnp.sum(acc_w, axis=0, keepdims=True)
        rd_w = exchange(0, send_w, recv_w)
        rd_w.start()

        strip.wait()
        acc_n = _chain_sum(
            [acc_n] + [nbuf[pl.ds(j * _RP, _RP), :] for j in range(ng)])
        part_n = jnp.sum(acc_n, axis=0, keepdims=True)
        send_n[...] = part_n
        rd_n = exchange(1, send_n, recv_n)
        rd_n.start()

        rd_w.wait_send()
        rd_n.wait_send()
        rd_w.wait_recv()
        out_ref[:, pl.ds(0, wide)] = send_w[...] + recv_w[...]
        rd_n.wait_recv()
        out_ref[:, pl.ds(wide, _NW)] = part_n + recv_n[...]

    return pl.pallas_call(
        body,
        out_shape=jax.ShapeDtypeStruct((1, n), jnp.float32),
        in_specs=[pl.BlockSpec(memory_space=pl.ANY)],
        out_specs=pl.BlockSpec(memory_space=pltpu.VMEM),
        scratch_shapes=[
            pltpu.VMEM((m, n), jnp.float32),
            pltpu.VMEM((srows, _NW), jnp.float32),
            pltpu.VMEM((1, wide), jnp.float32),
            pltpu.VMEM((1, wide), jnp.float32),
            pltpu.VMEM((1, _NW), jnp.float32),
            pltpu.VMEM((1, _NW), jnp.float32),
            pltpu.SemaphoreType.DMA((ng,)),
            pltpu.SemaphoreType.DMA((ng,)),
            pltpu.SemaphoreType.DMA,
            pltpu.SemaphoreType.DMA((2,)),
            pltpu.SemaphoreType.DMA((2,)),
        ],
        compiler_params=pltpu.CompilerParams(
            collective_id=0,
            disable_semaphore_checks=True,
            disable_bounds_checks=True,
        ),
    )(x)
```

```python
import jax
import jax.numpy as jnp
from jax import lax
from jax.experimental import pallas as pl
from jax.experimental.pallas import tpu as pltpu

_NS = 8
_RP = 8
_NW = 128
_DEPTH = 6
_CHAINS = 6
_TAIL = 4


def _chain_sum(parts):
    accs = list(parts[:_CHAINS])
    for i, p in enumerate(parts[_CHAINS:]):
        accs[i % _CHAINS] = accs[i % _CHAINS] + p
    while len(accs) > 1:
        nxt = [accs[i] + accs[i + 1] for i in range(0, len(accs) - 1, 2)]
        if len(accs) % 2:
            nxt.append(accs[-1])
        accs = nxt
    return accs[0]


def _aligned(v, k):
    return v if isinstance(v, int) else pl.multiple_of(v, k)


def pallas_dist_sum_ax0_xy_m2048_n1024_kernel(x: jax.Array):
    m, n = x.shape
    srows = m // _NS
    ng = srows // _RP
    nr = ng // 2
    gp = _NS - 1
    prows = gp * _RP
    grows = prows + _RP
    wide = n - _NW
    assert m % (2 * _NS * _RP) == 0 and wide == gp * _NW
    depth = min(_DEPTH, nr)

    def body(x_hbm, out_ref, buf, nbuf, send_w, recv_w, send_n, recv_n,
             sems_p, sems_t, strip_sems, send_sems, recv_sems):

        def fetch(row, slot, c0, w, sem, priority):
            pltpu.make_async_copy(
                x_hbm.at[pl.ds(row, _RP), pl.ds(c0, w)],
                buf.at[pl.ds(slot, _RP), pl.ds(c0, w)],
                sem,
            ).start(priority=priority)

        def issue(r, c, first=False):
            for j in range(2 * gp):
                g, i = 2 * r + j // gp, j % gp
                base = _aligned(g * grows, grows)
                t_row = (0 if first and j < gp
                         else _aligned(gp * srows + g * _RP, _RP))
                fetch(t_row, base + prows, i * _NW, _NW, sems_t.at[g], 0)
                p_row = _aligned((j // 2) * srows + (2 * r + j % 2) * _RP, _RP)
                fetch(p_row, base + i * _RP, wide, _NW, sems_p.at[g], 1)
                fetch(p_row + _RP, base + i * _RP, 0, wide, sems_p.at[g], 1)
            return c

        def consume(g, carry):
            acc_w, acc_n = carry
            base = pl.multiple_of(g * grows, grows)
            tiles = buf.at[pl.ds(base + prows, _RP), pl.ds(0, wide)]
            pltpu.make_async_copy(tiles, tiles, sems_t.at[g]).wait()
            pieces = buf.at[pl.ds(base, prows), :]
            pltpu.make_async_copy(pieces, pieces, sems_p.at[g]).wait()
            blk_w = buf[pl.ds(base, grows), pl.ds(0, wide)]
            blk_n = buf[pl.ds(base, prows), pl.ds(wide, _NW)]
            acc_w = acc_w + blk_w.reshape(gp + 1, _RP, wide).sum(axis=0)
            acc_n = acc_n + blk_n.reshape(gp, _RP, _NW).sum(axis=0)
            return acc_w, acc_n

        issue(0, 0, first=True)

        peer = (1 - lax.axis_index("x"), lax.axis_index("y"))
        bar = pltpu.get_barrier_semaphore()
        pl.semaphore_signal(bar, inc=1, device_id=peer,
                            device_id_type=pl.DeviceIdType.MESH)

        lax.fori_loop(1, depth, issue, 0)

        def steady(r, carry):
            issue(r + depth, 0)
            return consume(2 * r + 1, consume(2 * r, carry))

        carry = (jnp.zeros((_RP, wide), jnp.float32),
                 jnp.zeros((_RP, _NW), jnp.float32))
        carry = lax.fori_loop(0, nr - depth, steady, carry)

        strip_parts = ((0, ng - _TAIL), (ng - _TAIL, ng))
        strips = [
            pltpu.make_async_copy(
                x_hbm.at[pl.ds(m - srows + lo * _RP, (hi - lo) * _RP),
                         pl.ds(wide, _NW)],
                nbuf.at[pl.ds(lo * _RP, (hi - lo) * _RP), :],
                strip_sems.at[k])
            for k, (lo, hi) in enumerate(strip_parts)]
        for strip in strips:
            strip.start(priority=1)

        pl.semaphore_wait(bar, 1)

        def exchange(k, src, dst):
            return pltpu.make_async_remote_copy(
                src_ref=src, dst_ref=dst,
                send_sem=send_sems.at[k], recv_sem=recv_sems.at[k],
                device_id=peer, device_id_type=pl.DeviceIdType.MESH,
            )

        acc_w, acc_n = lax.fori_loop(2 * (nr - depth), ng, consume, carry)
        send_w[...] = jnp.sum(acc_w, axis=0, keepdims=True)
        rd_w = exchange(0, send_w, recv_w)
        rd_w.start()

        for strip, (lo, hi) in zip(strips, strip_parts):
            strip.wait()
            acc_n = _chain_sum(
                [acc_n]
                + [nbuf[pl.ds(j * _RP, _RP), :] for j in range(lo, hi)])
        part_n = jnp.sum(acc_n, axis=0, keepdims=True)
        send_n[...] = part_n
        rd_n = exchange(1, send_n, recv_n)
        rd_n.start()

        rd_w.wait_send()
        rd_n.wait_send()
        rd_w.wait_recv()
        out_ref[:, pl.ds(0, wide)] = send_w[...] + recv_w[...]
        rd_n.wait_recv()
        out_ref[:, pl.ds(wide, _NW)] = part_n + recv_n[...]

    return pl.pallas_call(
        body,
        out_shape=jax.ShapeDtypeStruct((1, n), jnp.float32),
        in_specs=[pl.BlockSpec(memory_space=pl.ANY)],
        out_specs=pl.BlockSpec(memory_space=pltpu.VMEM),
        scratch_shapes=[
            pltpu.VMEM((ng * grows, n), jnp.float32),
            pltpu.VMEM((srows, _NW), jnp.float32),
            pltpu.VMEM((1, wide), jnp.float32),
            pltpu.VMEM((1, wide), jnp.float32),
            pltpu.VMEM((1, _NW), jnp.float32),
            pltpu.VMEM((1, _NW), jnp.float32),
            pltpu.SemaphoreType.DMA((ng,)),
            pltpu.SemaphoreType.DMA((ng,)),
            pltpu.SemaphoreType.DMA((2,)),
            pltpu.SemaphoreType.DMA((2,)),
            pltpu.SemaphoreType.DMA((2,)),
        ],
        compiler_params=pltpu.CompilerParams(
            collective_id=0,
            disable_semaphore_checks=True,
        ),
    )(x)
```
